```python
import numpy as np

kernel_name = "dist_max_ax1_xy_m4096_n1024"

def setup_inputs():
    return {"x": np.random.randn(8192, 2048).astype(np.float32)}

def reference(x: np.ndarray) -> np.ndarray:
    return np.max(x, axis=1, keepdims=True)
```

```python
import jax
import jax.numpy as jnp
from jax import lax
from jax.experimental import pallas as pl
from jax.experimental.pallas import tpu as pltpu

_SHIFT = 1
_LAG = 46
_STEP = 4
_RING = 128
_SPLIT = ((8,), (2, 2, 2, 2))
_BATCHES = ((1, 24), (24, 32))
_TAIL = (11, 4)


def pallas_dist_max_ax1_xy_m4096_n1024_kernel(x: jax.Array):
    m, n = x.shape
    assert (m, n) == (4096, 1024)
    tiles = m // 8 * (n // 128)
    blocks = m // 128
    streams = blocks - 1
    n_main = streams * 16
    n_units = tiles // 8
    first, last = 128 - _SHIFT, tiles - 8 - _SHIFT
    lead = _LAG + streams + 1
    done = n_units - lead

    def unit_tile(u):
        if u <= n_main:
            return first + 128 * ((u - 1) % streams) + 8 * ((u - 1) // streams)
        return 8 * (u - n_main) - _SHIFT

    def next_tile(t):
        t = t + 128
        return jnp.where(t > last, t - (streams * 128 - 8), t)

    def body(x_hbm, o_ref, xv, acc, own, rcv, own0, rcv0, sems, send_sems, recv_sems):
        def fetch(t, size, u):
            return pltpu.make_async_copy(
                x_hbm.at[pl.ds(t, size)], xv.at[pl.ds(t, size)], sems.at[u & (_RING - 1)]
            )

        def start(u, t, queue):
            off = 0
            for size in _SPLIT[queue]:
                fetch(t + off, size, u).start(priority=queue)
                off += size

        def wait(u, t):
            fetch(t, 8, u).wait()

        def issue(u, t, count):
            for j in range(count):
                tail = 8 * (u + j - n_main) - _SHIFT
                start(u + j, jnp.where(u + j > n_main, tail, t), j % 2)
                t = next_tile(t)
            return t

        def fold(t):
            v = xv[pl.ds(t, 8)]
            vs = [v[i] for i in range(8)]
            while len(vs) > 1:
                vs = [jnp.maximum(vs[i], vs[i + 1]) for i in range(0, len(vs), 2)]
            return vs[0]

        def lane_max(v):
            return jnp.max(v, axis=1, keepdims=True)

        ends = [fetch(0, 8 - _SHIFT, 0), fetch(tiles - _SHIFT, _SHIFT, 0)]
        ends[0].start()
        start(1, first, 1)
        ends[1].start()
        t_issue = lax.fori_loop(
            1, lead // 2, lambda i, t: issue(2 * i, t, 2), jnp.int32(unit_tile(2))
        )

        peer = (lax.axis_index("x"), 1 - lax.axis_index("y"))
        barrier = pltpu.get_barrier_semaphore()
        pl.semaphore_signal(
            barrier, inc=1, device_id=peer, device_id_type=pl.DeviceIdType.MESH
        )

        def exchange(src, dst, i):
            copy = pltpu.make_async_remote_copy(
                src, dst, send_sems.at[i], recv_sems.at[i],
                device_id=peer, device_id_type=pl.DeviceIdType.MESH,
            )
            copy.start()
            return copy

        for end in ends:
            end.wait()
        neg_inf = jnp.full((8, 128), -jnp.inf, x.dtype)

        def first_round(b, _):
            acc[b] = neg_inf
            wait(b, first + 128 * (b - 1))

        lax.fori_loop(1, blocks, first_round, None)

        diag = lax.broadcasted_iota(jnp.int32, (8, 128), 1) - lax.broadcasted_iota(
            jnp.int32, (8, 128), 0
        )

        def steady(u, carry, count):
            t_issue, t_reduce = carry
            groups = []
            for j in range(count):
                wait(u + j - _LAG, t_reduce + 8)
                groups.append(t_reduce + _SHIFT)
                t_reduce = next_tile(t_reduce)
            maxes = [lane_max(fold(g)) for g in groups]
            t_issue = issue(u, t_issue, count)
            for g, q in zip(groups, maxes):
                pltpu.store(
                    acc.at[g >> 7], jnp.broadcast_to(q, (8, 128)), mask=diag == (g & 127)
                )
            return t_issue, t_reduce

        steps, rem = divmod(done, _STEP)
        carry = (t_issue, jnp.int32(first))
        if rem:
            carry = steady(lead, carry, rem)
        lax.fori_loop(
            0, steps, lambda i, c: steady(lead + rem + i * _STEP, c, _STEP), carry
        )

        pl.semaphore_wait(barrier, 1)
        sent = []
        for i, (lo, hi) in enumerate(_BATCHES):
            for u in range(done + streams + 1, n_main + 1):
                if lo <= (u - 1) % streams + 1 < hi:
                    wait(u, unit_tile(u))
            rows = []
            for b in range(lo, hi):
                a = acc[b]
                for k in range(16):
                    if k * streams + b > done:
                        a = jnp.where(diag == 8 * k, lane_max(fold(128 * b + 8 * k)), a)
                rows.append(jnp.max(a, axis=0, keepdims=True))
            if lo == 1:
                lo, rows = 0, [rows[0]] + rows
            span = pl.ds(lo, hi - lo)
            own[span] = jnp.concatenate(rows, axis=0)
            sent.append(exchange(own.at[span], rcv.at[span], i))

        a = neg_inf
        k = 0
        for count in _TAIL:
            folded = []
            for j in range(k, k + count):
                wait(n_main + 1 + j, unit_tile(n_main + 1 + j))
                folded += [(g, fold(8 * g)) for g in ([j] if j < 14 else [14, 15])]
            for g, v in folded:
                a = jnp.where(diag == 8 * g, lane_max(v), a)
            k += count
        row0 = jnp.max(a, axis=0, keepdims=True)
        own0[...] = row0
        final = exchange(own0, rcv0, len(_BATCHES))

        for copy in sent:
            copy.wait()
        o_ref[...] = jnp.maximum(own[...], rcv[...])
        final.wait()
        o_ref[pl.ds(0, 1), :] = jnp.maximum(row0, rcv0[...])

    x_tiles = (
        x.reshape(m // 8, 8, n // 128, 128).transpose(0, 2, 1, 3).reshape(tiles, 8, 128)
    )
    n_msgs = len(_BATCHES) + 1
    out = pl.pallas_call(
        body,
        out_shape=jax.ShapeDtypeStruct((blocks, 128), x.dtype),
        in_specs=[pl.BlockSpec(memory_space=pltpu.HBM)],
        out_specs=pl.BlockSpec(memory_space=pltpu.VMEM),
        scratch_shapes=[
            pltpu.VMEM((tiles, 8, 128), x.dtype),
            pltpu.VMEM((blocks, 8, 128), x.dtype),
            pltpu.VMEM((blocks, 128), x.dtype),
            pltpu.VMEM((blocks, 128), x.dtype),
            pltpu.VMEM((1, 128), x.dtype),
            pltpu.VMEM((1, 128), x.dtype),
            pltpu.SemaphoreType.DMA((_RING,)),
            pltpu.SemaphoreType.DMA((n_msgs,)),
            pltpu.SemaphoreType.DMA((n_msgs,)),
        ],
        compiler_params=pltpu.CompilerParams(
            collective_id=0,
            vmem_limit_bytes=24 * 1024 * 1024,
            disable_bounds_checks=True,
            disable_semaphore_checks=True,
        ),
    )(x_tiles)
    return out.reshape(m, 1)
```

```python
import jax
import jax.numpy as jnp
from jax import lax
from jax.experimental import pallas as pl
from jax.experimental.pallas import tpu as pltpu

_SKEW = 128
_CUTS = ((896,), (384, 256, 256))
_LAG = 48
_RING = 64
_STEP = 4
_TAIL_FROM = (502, 493)
_BATCHES = ((1, 24), (24, 32))
_STAGES = ((0, 6), (6, 16))


def pallas_dist_max_ax1_xy_m4096_n1024_kernel(x: jax.Array):
    m, n = x.shape
    assert (m, n) == (4096, 1024)
    groups, blocks = m // 8, m // 128

    main = [0] + [16 * b + k for k in range(16) for b in range(1, blocks)]
    tail = list(range(1, 16))
    order = [(tail if s >= _TAIL_FROM[s % 2] else main).pop(0) for s in range(groups)]

    def following(p):
        return jnp.where(p >= groups - 16, p - groups + 33, p + 16)

    def body(x_hbm, o_ref, buf, acc, own, got, own0, got0, sems, send_sems, recv_sems):
        def start(s, p, queue):
            def copy(g, src_col, dst_col, width):
                pltpu.make_async_copy(
                    x_hbm.at[g, :, pl.ds(src_col, width)],
                    buf.at[p, :, pl.ds(dst_col, width)],
                    sems.at[s & (_RING - 1)],
                ).start(priority=queue)

            copy((p - 1) & (groups - 1), n - _SKEW, 0, _SKEW)
            col = 0
            for width in _CUTS[queue]:
                copy(p, col, _SKEW + col, width)
                col += width

        def wait(s, p):
            pltpu.make_async_copy(buf.at[p], buf.at[p], sems.at[s & (_RING - 1)]).wait()

        def fold(g):
            parts = (buf[g, :, _SKEW:], buf[(g + 1) & (groups - 1), :, :_SKEW])
            vs = [v[:, c : c + 128] for v in parts for c in range(0, v.shape[1], 128)]
            while len(vs) > 1:
                vs = [jnp.maximum(a, b) for a, b in zip(vs[0::2], vs[1::2])]
            return vs[0]

        def lane_max(v):
            return jnp.max(v, axis=1, keepdims=True)

        neg_inf = jnp.full((8, 128), -jnp.inf, x.dtype)
        lane = lax.broadcasted_iota(jnp.int32, (8, 128), 1)
        diagonal = lane - lax.broadcasted_iota(jnp.int32, (8, 128), 0)

        def place(g, row_max, tile):
            return jnp.where(diagonal == 8 * (g & 15), row_max, tile)

        def fill(i, p):
            for queue in range(2):
                start(2 * i + queue, p, queue)
                p = following(p)
            return p

        def prime(i, p):
            for b in (2 * i, 2 * i + 1):
                wait(b, 16 * b)
                acc[b] = neg_inf
            return fill(i + _LAG // 2, p)

        def steady(i, carry):
            p, p_tail, landed = carry
            s = _LAG + blocks + i * _STEP
            ready = []
            for j in range(_STEP):
                wait(s + j - _LAG, landed)
                ready.append(landed - 1)
                landed = following(landed)
            maxes = [lane_max(fold(g)) for g in ready]
            for j in range(_STEP):
                is_tail = s + j >= _TAIL_FROM[j % 2]
                start(s + j, jnp.where(is_tail, p_tail, p), j % 2)
                p = jnp.where(is_tail, p, following(p))
                p_tail = jnp.where(is_tail, p_tail + 1, p_tail)
            for g, row_max in zip(ready, maxes):
                acc[g >> 4] = place(g, row_max, acc[g >> 4])
            return p, p_tail, landed

        p = lax.fori_loop(0, _LAG // 2, fill, jnp.int32(0))
        peer = (lax.axis_index("x"), 1 - lax.axis_index("y"))
        barrier = pltpu.get_barrier_semaphore()
        pl.semaphore_signal(
            barrier, inc=1, device_id=peer, device_id_type=pl.DeviceIdType.MESH
        )
        p = lax.fori_loop(0, blocks // 2, prime, p)
        lax.fori_loop(
            0,
            (groups - _LAG - blocks) // _STEP,
            steady,
            (p, jnp.int32(1), jnp.int32(order[blocks])),
        )

        in_flight = order[groups - _LAG :]
        reduced = [u - 1 for u in order[blocks : groups - _LAG]]

        def wait_for_group(g):
            for u in (g, (g + 1) % groups):
                if u in in_flight:
                    wait(order.index(u), u)
                    in_flight.remove(u)

        def exchange(src, dst, i):
            copy = pltpu.make_async_remote_copy(
                src,
                dst,
                send_sems.at[i],
                recv_sems.at[i],
                device_id=peer,
                device_id_type=pl.DeviceIdType.MESH,
            )
            copy.start()
            return copy

        pl.semaphore_wait(barrier, 1)
        sent = []
        for i, (lo, hi) in enumerate(_BATCHES):
            todo = [g for g in range(16 * lo, 16 * hi) if g not in reduced]
            for g in todo:
                wait_for_group(g)
            lo -= lo % 8
            tiles = [acc[b] for b in range(lo, hi)]
            for g in todo:
                tiles[g // 16 - lo] = place(g, lane_max(fold(g)), tiles[g // 16 - lo])
            span = pl.ds(lo, hi - lo)
            own[span] = jnp.concatenate(
                [jnp.max(tile, axis=0, keepdims=True) for tile in tiles]
            )
            sent.append(exchange(own.at[span], got.at[span], i))

        tile = neg_inf
        for lo, hi in _STAGES:
            folded = []
            for g in range(lo, hi):
                wait_for_group(g)
                folded.append(fold(g))
            for g, v in zip(range(lo, hi), folded):
                tile = place(g, lane_max(v), tile)
        assert not in_flight
        row0 = jnp.max(tile, axis=0, keepdims=True)
        own0[...] = row0
        last = exchange(own0, got0, len(_BATCHES))

        for copy in sent:
            copy.wait()
        o_ref[...] = jnp.maximum(own[...], got[...])
        last.wait()
        o_ref[pl.ds(0, 1), :] = jnp.maximum(row0, got0[...])

    messages = len(_BATCHES) + 1
    out = pl.pallas_call(
        body,
        out_shape=jax.ShapeDtypeStruct((blocks, 128), x.dtype),
        in_specs=[pl.BlockSpec(memory_space=pltpu.HBM)],
        out_specs=pl.BlockSpec(memory_space=pltpu.VMEM),
        scratch_shapes=[
            pltpu.VMEM((groups, 8, n), x.dtype),
            pltpu.VMEM((blocks, 8, 128), x.dtype),
            pltpu.VMEM((blocks, 128), x.dtype),
            pltpu.VMEM((blocks, 128), x.dtype),
            pltpu.VMEM((1, 128), x.dtype),
            pltpu.VMEM((1, 128), x.dtype),
            pltpu.SemaphoreType.DMA((_RING,)),
            pltpu.SemaphoreType.DMA((messages,)),
            pltpu.SemaphoreType.DMA((messages,)),
        ],
        compiler_params=pltpu.CompilerParams(
            collective_id=0,
            vmem_limit_bytes=24 * 1024 * 1024,
            disable_bounds_checks=True,
            disable_semaphore_checks=True,
        ),
    )(x.reshape(groups, 8, n))
    return out.reshape(m, 1)
```
